```python
import numpy as np

kernel_name = "dist_sum_ax1_xy_m512_n256"

def setup_inputs():
    return {"x": np.random.randn(1024, 512).astype(np.float32)}

def reference(x: np.ndarray) -> np.ndarray:
    return np.sum(x, axis=1, keepdims=True)
```

```python
import jax
import jax.numpy as jnp
from jax import lax
from jax.experimental import pallas as pl
from jax.experimental.pallas import tpu as pltpu

_CHUNKS = (384, 128)


def pallas_dist_sum_ax1_xy_m512_n256_kernel(
x: jax.Array,
):
    m, n = x.shape
    sizes = _CHUNKS if sum(_CHUNKS) == m else (m,)
    offs = [sum(sizes[:i]) for i in range(len(sizes))]
    nc = len(sizes)

    def body(x_hbm, out_ref, xbuf, send_buf, recv_buf, in_sems, send_sems, recv_sems):
        loads = []
        for c in range(nc):
            rows = pl.ds(offs[c], sizes[c])
            cp = pltpu.make_async_copy(x_hbm.at[rows], xbuf.at[rows], in_sems.at[c])
            cp.start()
            loads.append(cp)

        peer = (lax.axis_index("x"), 1 - lax.axis_index("y"))
        barrier = pltpu.get_barrier_semaphore()
        pl.semaphore_signal(
            barrier, inc=1, device_id=peer, device_id_type=pl.DeviceIdType.MESH
        )

        rdmas = []
        for c in range(nc):
            cols = pl.ds(offs[c], sizes[c])
            loads[c].wait()
            xv = xbuf[pl.ds(offs[c], sizes[c]), :]
            acc = xv[:, 0:128]
            for j in range(1, n // 128):
                acc = acc + xv[:, j * 128:(j + 1) * 128]
            send_buf[:, cols] = jnp.sum(acc, axis=1).reshape(1, sizes[c])
            if c == 0:
                pl.semaphore_wait(barrier, 1)
            rdma = pltpu.make_async_remote_copy(
                src_ref=send_buf.at[:, cols],
                dst_ref=recv_buf.at[:, cols],
                send_sem=send_sems.at[c],
                recv_sem=recv_sems.at[c],
                device_id=peer,
                device_id_type=pl.DeviceIdType.MESH,
            )
            rdma.start()
            rdmas.append(rdma)

        for c in range(nc):
            rdmas[c].wait_send()
        for c in range(nc):
            cols = pl.ds(offs[c], sizes[c])
            rdmas[c].wait_recv()
            out_ref[:, cols] = send_buf[:, cols] + recv_buf[:, cols]

    out = pl.pallas_call(
        body,
        out_shape=jax.ShapeDtypeStruct((1, m), x.dtype),
        in_specs=[pl.BlockSpec(memory_space=pl.ANY)],
        out_specs=pl.BlockSpec(memory_space=pltpu.VMEM),
        scratch_shapes=[
            pltpu.VMEM((m, n), x.dtype),
            pltpu.VMEM((1, m), x.dtype),
            pltpu.VMEM((1, m), x.dtype),
            pltpu.SemaphoreType.DMA((nc,)),
            pltpu.SemaphoreType.DMA((nc,)),
            pltpu.SemaphoreType.DMA((nc,)),
        ],
        compiler_params=pltpu.CompilerParams(
            collective_id=0,
            disable_bounds_checks=True,
            disable_semaphore_checks=True,
        ),
    )(x)
    return out.reshape(m, 1)
```

```python
import jax
import jax.numpy as jnp
from jax import lax
from jax.experimental import pallas as pl
from jax.experimental.pallas import tpu as pltpu

_LANES = 128
_TAIL_ROWS = 128


def pallas_dist_sum_ax1_xy_m512_n256_kernel(
x: jax.Array,
):
    m, n = x.shape
    sizes = (m - _TAIL_ROWS, _TAIL_ROWS)
    offs = (0, m - _TAIL_ROWS)
    nc = len(sizes)

    def body(x_hbm, out_ref, *scratch):
        x_bufs = scratch[0:nc]
        send_bufs = scratch[nc:2 * nc]
        recv_bufs = scratch[2 * nc:3 * nc]
        load_sems, send_sems, recv_sems = scratch[3 * nc:]

        loads = []
        for c in range(nc):
            cp = pltpu.make_async_copy(
                x_hbm.at[pl.ds(offs[c], sizes[c])], x_bufs[c], load_sems.at[c]
            )
            cp.start()
            loads.append(cp)

        peer = (lax.axis_index("x"), 1 - lax.axis_index("y"))
        barrier = pltpu.get_barrier_semaphore()
        pl.semaphore_signal(
            barrier, inc=1, device_id=peer, device_id_type=pl.DeviceIdType.MESH
        )

        rdmas = []
        for c in range(nc):
            loads[c].wait()
            xv = x_bufs[c][...]
            acc = xv[:, 0:_LANES]
            for j in range(1, n // _LANES):
                acc = acc + xv[:, j * _LANES:(j + 1) * _LANES]
            send_bufs[c][...] = jnp.sum(acc, axis=1).reshape(1, sizes[c])
            if c == 0:
                pl.semaphore_wait(barrier, 1)
            rdma = pltpu.make_async_remote_copy(
                src_ref=send_bufs[c],
                dst_ref=recv_bufs[c],
                send_sem=send_sems.at[c],
                recv_sem=recv_sems.at[c],
                device_id=peer,
                device_id_type=pl.DeviceIdType.MESH,
            )
            rdma.start()
            rdmas.append(rdma)

        for c in range(nc):
            rdmas[c].wait_send()
        for c in range(nc):
            rdmas[c].wait_recv()
            out_ref[:, pl.ds(offs[c], sizes[c])] = send_bufs[c][...] + recv_bufs[c][...]

    out = pl.pallas_call(
        body,
        out_shape=jax.ShapeDtypeStruct((1, m), x.dtype),
        in_specs=[pl.BlockSpec(memory_space=pl.ANY)],
        out_specs=pl.BlockSpec(memory_space=pltpu.VMEM),
        scratch_shapes=(
            [pltpu.VMEM((s, n), x.dtype) for s in sizes]
            + [pltpu.VMEM((1, s), x.dtype) for s in sizes]
            + [pltpu.VMEM((1, s), x.dtype) for s in sizes]
            + [pltpu.SemaphoreType.DMA((nc,)) for _ in range(3)]
        ),
        compiler_params=pltpu.CompilerParams(
            collective_id=0,
            disable_bounds_checks=True,
            disable_semaphore_checks=True,
        ),
    )(x)
    return out.reshape(m, 1)
```

```python
import jax
import jax.numpy as jnp
from jax import lax
from jax.experimental import pallas as pl
from jax.experimental.pallas import tpu as pltpu

_LANES = 128
_TAIL_CHUNKS = (128, 96)
_TAIL_MSG = 128


def _offsets(sizes):
    return [sum(sizes[:i]) for i in range(len(sizes))]


def pallas_dist_sum_ax1_xy_m512_n256_kernel(
x: jax.Array,
):
    m, n = x.shape
    chunks = (m - sum(_TAIL_CHUNKS),) + _TAIL_CHUNKS
    msgs = (m - _TAIL_MSG, _TAIL_MSG)
    chunk_offs, msg_offs = _offsets(chunks), _offsets(msgs)
    nc, nm = len(chunks), len(msgs)

    def body(x_hbm, out_ref, *scratch):
        x_bufs = scratch[:nc]
        send_bufs = scratch[nc:nc + nm]
        recv_bufs = scratch[nc + nm:nc + 2 * nm]
        load_sems, send_sems, recv_sems = scratch[nc + 2 * nm:]

        loads = []
        for c in range(nc):
            cp = pltpu.make_async_copy(
                x_hbm.at[pl.ds(chunk_offs[c], chunks[c])], x_bufs[c], load_sems.at[c]
            )
            cp.start()
            loads.append(cp)

        peer = (lax.axis_index("x"), 1 - lax.axis_index("y"))
        barrier = pltpu.get_barrier_semaphore()
        pl.semaphore_signal(
            barrier, inc=1, device_id=peer, device_id_type=pl.DeviceIdType.MESH
        )

        rdmas = []
        for c in range(nc):
            loads[c].wait()
            xv = x_bufs[c][...]
            acc = xv[:, 0:_LANES]
            for j in range(1, n // _LANES):
                acc = acc + xv[:, j * _LANES:(j + 1) * _LANES]
            lo, hi = chunk_offs[c], chunk_offs[c] + chunks[c]
            for k in range(nm):
                a = max(lo, msg_offs[k])
                b = min(hi, msg_offs[k] + msgs[k])
                if a < b:
                    sums = jnp.sum(acc[a - lo:b - lo], axis=1).reshape(1, b - a)
                    send_bufs[k][:, pl.ds(a - msg_offs[k], b - a)] = sums
            while len(rdmas) < nm and msg_offs[len(rdmas)] + msgs[len(rdmas)] <= hi:
                k = len(rdmas)
                if k == 0:
                    pl.semaphore_wait(barrier, 1)
                rdma = pltpu.make_async_remote_copy(
                    src_ref=send_bufs[k],
                    dst_ref=recv_bufs[k],
                    send_sem=send_sems.at[k],
                    recv_sem=recv_sems.at[k],
                    device_id=peer,
                    device_id_type=pl.DeviceIdType.MESH,
                )
                rdma.start()
                rdmas.append(rdma)

        for k in range(nm):
            rdmas[k].wait_send()
        for k in range(nm):
            rdmas[k].wait_recv()
            out_ref[:, pl.ds(msg_offs[k], msgs[k])] = (
                send_bufs[k][...] + recv_bufs[k][...]
            )

    out = pl.pallas_call(
        body,
        out_shape=jax.ShapeDtypeStruct((1, m), x.dtype),
        in_specs=[pl.BlockSpec(memory_space=pl.ANY)],
        out_specs=pl.BlockSpec(memory_space=pltpu.VMEM),
        scratch_shapes=(
            [pltpu.VMEM((s, n), x.dtype) for s in chunks]
            + [pltpu.VMEM((1, s), x.dtype) for s in msgs]
            + [pltpu.VMEM((1, s), x.dtype) for s in msgs]
            + [
                pltpu.SemaphoreType.DMA((nc,)),
                pltpu.SemaphoreType.DMA((nm,)),
                pltpu.SemaphoreType.DMA((nm,)),
            ]
        ),
        compiler_params=pltpu.CompilerParams(
            collective_id=0,
            disable_semaphore_checks=True,
        ),
    )(x)
    return out.reshape(m, 1)
```
